```python
import numpy as np

kernel_name = "dist_sparse_attn_localglobal_htp_kvseq_b2_sq256_skv256_hq4_dh64"

def setup_inputs():
    x = np.random.randn(2, 256, 512).astype(np.float32)
    Wq = np.random.randn(512, 1024).astype(np.float32) * 0.02
    K_ext = np.random.randn(2, 1024, 16, 64).astype(np.float32)
    V_ext = np.random.randn(2, 1024, 16, 64).astype(np.float32)
    Wo = np.random.randn(1024, 512).astype(np.float32) * 0.02
    return {"x": x, "Wq": Wq, "K_ext": K_ext, "V_ext": V_ext, "Wo": Wo}

def reference(x, Wq, K_ext, V_ext, Wo):
    B, Sq, Skv, Hq, Dh = 2, 256, 1024, 16, 64
    Q = (x @ Wq).reshape(B, Sq, Hq, Dh)
    qi = np.arange(Sq)[:, None]
    ki = np.arange(Skv)[None, :]
    local = np.abs(qi - ki) <= 128
    glob = (ki < 32) | (qi < 32)
    mask = local | glob
    scores = np.einsum('bihd,bjhd->bhij', Q, K_ext).astype(np.float32) * 0.125
    scores = np.where(mask[None, None, :, :], scores, -1e9)
    scores_max = scores.max(axis=-1, keepdims=True)
    w = np.exp(scores - scores_max)
    row_keep = mask.any(axis=1)
    w_sum = np.where(row_keep[None, None, :, None], w.sum(axis=-1, keepdims=True), 1.0)
    w = w / w_sum
    w = np.where(row_keep[None, None, :, None], w, 0.0)
    ctx = np.einsum('bhij,bjhd->bihd', w, V_ext).reshape(B, Sq, Hq * Dh)
    return ctx @ Wo
```

```python
import jax
import jax.numpy as jnp
from jax import lax
from jax.experimental import pallas as pl
from jax.experimental.pallas import tpu as pltpu

F32 = jnp.float32
BF16 = jnp.bfloat16
LOG2E = 1.4426950408889634
SCALE = 0.125 * LOG2E
NEG = -1e9 * LOG2E
NT = (((1,), (1,)), ((), ()))
MESH = pl.DeviceIdType.MESH
DEPTH = 3
CODE_ORDER = (3, 1, 2, 0)

HOME = [0, 0, 1, 1, 2, 3, 0, 0]
MAIN = [[0, 0], [0, 0], [0, 1], [1, 1], [2, 2], [3, 3], [0, 0], [0, 0]]
TRI = [[0, 0], [0, 0], [1, 1], [1, 1], [2, 2], [1, 3], [0, 0], [1, 1]]
OUT = [[0, 0], [0, 0], [1, 1], [1, 1], [1, 2], [1, 3], [0, 0], [0, 0]]
G_OUT = [0, 0, 1, 1, 1, 1, 0, 0]
Q_TO_TRI = {5: [(2, 1)], 7: [(3, 2), (2, 1)]}
TRI_PATH = {(5, 1): [(1, 2), (2, 3)]}
MERGE_AT = {(5, 0, "T"): 1}
BACK = {(5, 0, "T"): [(3, 2), (2, 1)]}
CTX_PATH = {(5, 0): [(3, 2), (2, 1)], (4, 0): [(2, 1)]}
WQ_ROWS = {5: (0, 64, 256, 512), 6: (0, 16, 64, 256, 512), 7: (0, 256, 400, 512)}
FIRST_TRI = (0, 0)
W_DETOUR = {"Wq7h2": [(3, 2), (2, 1), (1, 0)]}
KV_DETOUR = {"K40": (80, [(0, 1), (1, 2)])}
V_LAST = [(5, 1)]
QG_TREE = {
    0: [((0, 1), [(0, 1), (1, 2), (2, 3)])],
    1: [((0, 1), [(1, 2), (2, 3)])],
    2: [((0, 1), [(2, 1)]), ((0,), [(2, 3)])],
    3: [((0, 1), [(3, 2), (2, 1)])],
}
CG_PATH = {0: [(1, 2), (2, 3), (3, 0)], 1: [(3, 2), (2, 1)]}
LOADS = [
    [("xg", "x", (0, 2), (0, 32)), ("x0", "x", (0, 1), (32, 256)),
     ("x1", "x", (1, 2), (32, 256)), ("Wq", "wq"), ("Wo", "wo"), ("K31", "k", (1, 2), (3, 4)),
     ("V31", "v", (1, 2), (3, 4)), ("K50", "k", (0, 1), (5, 6)), ("V50", "v", (0, 1), (5, 6)),
     ("K21", "k", (1, 2), (2, 3)), ("V21", "v", (1, 2), (2, 3)), ("K240", "k", (0, 1), (2, 5)),
     ("V240", "v", (0, 1), (2, 5)), ("K451", "k", (1, 2), (4, 6)), ("V451", "v", (1, 2), (4, 6)),
     ("Ka", "k", (0, 2), (0, 2)), ("Va", "v", (0, 2), (0, 2)), ("Kz", "k", (0, 2), (6, 8)),
     ("Vz", "v", (0, 2), (6, 8))],
    [("xg", "x", (0, 2), (0, 32)), ("x0", "x", (0, 1), (32, 256)),
     ("x1", "x", (1, 2), (32, 256)), ("Wq", "wq"), ("Wo", "wo"),
     ("Vt00", "v", (0, 1), (0, 1), (0, 128), (0, 128)),
     ("Kt13", "k", (0, 1), (1, 4), (0, 128), (0, 128)),
     ("Vt13", "v", (0, 1), (1, 4), (0, 128), (0, 128)),
     ("Kt40", "k", (0, 1), (4, 5), (0, 128), (0, 128)),
     ("Vt40", "v", (0, 1), (4, 5), (0, 128), (0, 128)),
     ("Kt57", "k", (0, 1), (5, 8), (0, 128), (0, 128)),
     ("Vt57", "v", (0, 1), (5, 8), (0, 128), (0, 128)),
     ("Kt1a", "k", (1, 2), (0, 4), (0, 128), (0, 128)),
     ("Vt1a", "v", (1, 2), (0, 4), (0, 128), (0, 128)),
     ("Kt1z", "k", (1, 2), (4, 8), (0, 128), (0, 128)),
     ("Vt1z", "v", (1, 2), (4, 8), (0, 128), (0, 128)),
     ("Ka00", "k", (0, 1), (0, 1), (0, 16), (0, 128)),
     ("Kt00", "k", (0, 1), (0, 1), (16, 128), (0, 128)),
     ("KrA", "k", (0, 2), (0, 2), (0, 128), (128, 256)),
     ("VrA", "v", (0, 2), (0, 2), (0, 128), (128, 256)),
     ("KrM", "k", (0, 2), (2, 6), (0, 128), (128, 256)),
     ("VrM", "v", (0, 2), (2, 6), (0, 128), (128, 256)),
     ("KrZ", "k", (0, 2), (6, 8), (0, 128), (128, 256)),
     ("VrZ", "v", (0, 2), (6, 8), (0, 128), (128, 256))],
    [("xg", "x", (0, 2), (0, 32)), ("x0", "x", (0, 1), (32, 256)),
     ("x1", "x", (1, 2), (32, 256)), ("Wq5h0", "wq", (0, 64), (128, 256)),
     ("Wq5h1", "wq", (64, 256), (128, 256)), ("Wq5h2", "wq", (256, 512), (128, 256)),
     ("Wq4", "wq", (0, 512), (0, 128)), ("Wo4h0", "wo", (0, 128), (0, 256)),
     ("Wo4h1", "wo", (0, 128), (256, 512)), ("Wo5", "wo", (128, 256)),
     ("Ko0", "k", (0, 2), (0, 2)), ("Vo0", "v", (0, 2), (0, 2)), ("Ko1", "k", (0, 2), (2, 4)),
     ("Vo1", "v", (0, 2), (2, 4)), ("Ko2", "k", (0, 2), (4, 6)), ("Vo2", "v", (0, 2), (4, 6)),
     ("Ko3", "k", (0, 2), (6, 8)), ("Vo3", "v", (0, 2), (6, 8))],
    [("xg", "x", (0, 2), (0, 32)), ("x0", "x", (0, 1), (32, 256)),
     ("x1", "x", (1, 2), (32, 256)), ("Wq6h0", "wq", (0, 16), (0, 128)),
     ("Wq6h1", "wq", (16, 64), (0, 128)), ("Wq6h2", "wq", (64, 256), (0, 128)),
     ("Wq6h3", "wq", (256, 512), (0, 128)), ("Wq7", "wq", (0, 512), (128, 256)), ("Wo", "wo"),
     ("Ko0", "k", (0, 2), (0, 2)), ("Vo0", "v", (0, 2), (0, 2)), ("Ko1", "k", (0, 2), (2, 4)),
     ("Vo1", "v", (0, 2), (2, 4)), ("Ko2", "k", (0, 2), (4, 6)), ("Vo2", "v", (0, 2), (4, 6)),
     ("Ko3", "k", (0, 2), (6, 8)), ("Vo3", "v", (0, 2), (6, 8))],
]
PATTERNS = [
    ([(0, 1, [-1]), (1, 0, [-1]), (1, 2, [-1, 0]), (2, 3, [2])],
     [[-1, 1], [-1, 0], [2], [3]]),
    ([(1, 0, [-1]), (0, 1, [-1]), (1, 2, [-1, 1]), (0, 3, [-1, 0])],
     [[-1, 0], [-1, 1], [2], [3]]),
    ([(0, 1, [-1]), (1, 2, [-1, 0]), (2, 3, [1]), (3, 0, [2])],
     [[3], [-1, 0], [1], [2]]),
    ([(1, 0, [-1]), (0, 3, [-1, 0]), (0, 1, [-1]), (3, 2, [1])],
     [[-1, 0], [-1, 2], [3], [1]]),
    ([(1, 0, [-1]), (0, 3, [-1, 0]), (3, 2, [1]), (0, 1, [-1])],
     [[-1, 0], [-1, 3], [2], [1]]),
    ([(0, 1, [-1]), (1, 2, [-1, 0]), (1, 0, [-1]), (2, 3, [1])],
     [[-1, 2], [-1, 0], [1], [3]]),
    ([(1, 0, [-1]), (0, 3, [-1, 0]), (0, 1, [-1]), (1, 2, [-1, 2])],
     [[-1, 0], [-1, 2], [3], [1]]),
    ([(0, 1, [-1]), (1, 2, [-1, 0]), (2, 3, [1]), (1, 0, [-1])],
     [[-1, 3], [-1, 0], [1], [2]]),
    ([(0, 1, [-1]), (1, 0, [-1]), (0, 3, [-1, 1]), (1, 2, [-1, 0])],
     [[-1, 1], [-1, 0], [3], [2]]),
    ([(0, 3, [-1]), (1, 2, [-1]), (3, 2, [-1, 0]), (2, 3, [-1, 1]), (3, 0, [-1, 3]),
      (2, 1, [-1, 2])],
     [[-1, 4], [-1, 5], [-1, 1, 2], [-1, 0, 3]]),
    ([(1, 2, [-1]), (0, 3, [-1]), (2, 3, [-1, 0]), (3, 2, [-1, 1]), (3, 0, [-1, 2]),
      (0, 1, [-1, 4])],
     [[-1, 4], [5], [-1, 0, 3], [-1, 1, 2]]),
    ([(0, 1, [-1]), (3, 2, [-1]), (1, 2, [-1, 0]), (2, 1, [-1, 1]), (2, 3, [-1, 2]),
      (3, 0, [-1, 4])],
     [[5], [-1, 0, 3], [-1, 1, 2], [-1, 4]]),
    ([(2, 1, [-1]), (3, 0, [-1]), (1, 0, [-1, 0]), (0, 1, [-1, 1]), (1, 2, [-1, 3]),
      (0, 3, [-1, 2])],
     [[-1, 1, 2], [-1, 0, 3], [-1, 4], [-1, 5]]),
]
ATOMS = {(0, 0, 32, 0): 0, (0, 0, 32, 1): 1, (0, 32, 64, 0): 0, (0, 32, 64, 1): 0,
         (0, 64, 96, 0): 2, (0, 64, 96, 1): 0, (0, 96, 128, 0): 2, (0, 96, 128, 1): 3,
         (0, 128, 160, 0): 4, (0, 128, 160, 1): 3, (0, 160, 192, 0): 5, (0, 160, 192, 1): 1,
         (0, 192, 208, 0): 6, (0, 192, 208, 1): 1, (0, 208, 224, 0): 1, (0, 208, 224, 1): 1,
         (0, 224, 240, 0): 0, (0, 224, 240, 1): 5, (0, 240, 256, 0): 7, (0, 240, 256, 1): 1,
         (1, 0, 32, 0): 0, (1, 0, 32, 1): 8, (1, 32, 64, 0): 9, (1, 32, 64, 1): 9,
         (1, 64, 96, 0): 9, (1, 64, 96, 1): 10, (1, 96, 128, 0): 9, (1, 96, 128, 1): 10,
         (1, 128, 160, 0): 9, (1, 128, 160, 1): 9, (1, 160, 192, 0): 9, (1, 160, 192, 1): 9,
         (1, 192, 208, 0): 9, (1, 192, 208, 1): 9, (1, 208, 224, 0): 9, (1, 208, 224, 1): 11,
         (1, 224, 240, 0): 9, (1, 224, 240, 1): 9, (1, 240, 256, 0): 12, (1, 240, 256, 1): 9}
ORDER = [
    """
    L0:K21 L0:K31 L0:V31 L0:K50 L0:xg L0:V50 L0:Wq L0:K240 L0:x0 L0:V240 L0:Va L0:K451 L0:x1
    L0:V21 L0:Ka L0:V451 L0:Vz L0:Kz L0:Wo cK21 cK31 cK50 K31@01 w:L0:xg w:L0:V31 w:L0:V50 K50@03
    cXg0 cV31 cV50 cWq1h1 cWq0h0 cWq1h0 V50@03 cK40 cWq0h1 Qg0 Qg0j01@01 cK20 K40x@01 V31@01
    K21@01 K40@02 cV40 V40@02 w:Wq6h0@30 w:Wq6h1@30 w:Wq6h2@30 w:L0:x0 cV11 cV01 s:K31@01
    s:K50@03 cK51 cV10 s:Qg0j01@01 cX01 Q61Ld0 Q01Ld0 cV21 cX00 Q00Td0 cK41 Q11Td0 Q10Ld0 K41@02
    Q01Td0 Q10Td0 cV00 cV30 V21@01 s:V50@03 s:K40x@01 s:V31@01 cV41 V41@02 cK10 A10L Q60Td0 cK00
    Q00Ld0 A00L cK01 A01L cK30 K30@01 w:L0:Vz w:Ka00@10 w:Kt00@10 w:Vt00@10 w:KVt01@10 w:Wq7h0@30
    K51@03 Q61Td0 cV70 w:Wq7h1@30 s:K21@01 s:K40@02 cK61 cK70 cV60 A00T A01T cWo0h0 s:V40@02
    Q70Td0 V30@01 w:Q20T@10 w:Q20L@10 cV71 Q11Ld0 Q71Ld0 cV20 cK60 A20T cK11 cV51 Q60Ld0 A20L
    A11L A60L cWo0h1 CX20L@01 V51@03 w:Wo6h0@30 CX20T@01 A11T E0 Q71Td0 cWo1h0 Q70Ld0 cV61 cK71
    A70L A61L A71L O0b1r64c0 ARb1r64c0m0@03 w:KVt61@10 O0b0r96c0 A61T cWo1h1 O0b1r32c0 O0b0r32c0
    O0b0r64c0 A70T A71T O0b1r96c0 MG71T ARb1r96c0m0@03 ARb0r64c0m0@01 O0b1r224c0 O0b1r192c0
    ARb1r208c0m0@03 ARb1r192c0m0@03 ARb1r224c0m0@03 ARb0r96c0m0@01 w:Wo6h1@30 ARb0r32c0m0@01
    s:K41@02 O0b0r96c1 O0b0r64c1 O0b1r160c1 O0b1r128c1 O0b1r192c1 O0b1r224c1 ARb1r224c1m0@03
    ARb1r128c1m0@03 O0b1r64c1 ARb1r208c1m0@01 ARb1r240c1m0@03 ARb0r96c1m2@01 ARb1r192c1m0@03
    w:KVt60@10 ARb0r64c1m0@01 A10T O0b1r32c1 O0b1r160c0 A60T O0b0r32c1 ARb1r160c0m0@03 MG70T
    ARb1r160c1m0@03 ARb0r32c1m0@01 O0b0r224c0 O0b0r224c1 O0b0r160c0 ARb0r224c1m0@01
    ARb0r160c0m0@01 ARb1r32c0m0@03 O0b0r160c1 O0b1r128c0 ARb1r32c1m0@03 w:ARb1r240c0m1@30
    ARb0r240c1m1@01 ARb1r240c0m3@01 ARb1r128c0m0@03 w:cg0b0@30 ARb0r224c0m0@01 OG0b0 w:cg0b1@30
    s:V21@01 s:V41@02 s:K30@01 s:K51@03 s:V30@01 s:CX20L@01 s:V51@03 s:CX20T@01 ARb0r96c1m1@03
    OG0b1 ARb0r240c0m0@01 O0b0r192c1 ARb0r0c0m0@01 ARb0r208c1m1@01 O0b0r192c0 ARb0r192c1m1@01
    ARb0r192c0m2@01 ARb0r160c1m3@03 w:ARb1r192c1m4@30 w:ARb1r192c0m4@30 ARb1r0c0m0@01 F0b1r192c1
    F0b1r192c0 ARb1r64c1m1@03 ARb0r160c1m1@01 ARb0r0c1m1@01 O0b1r96c1 ARb1r96c1m1@03 F0b0r32c1
    O0b0r128c0 ARb0r240c1m3@03 ARb0r208c0m1@01 w:ARb0r208c0m0@10 ARb1r64c1m5@01 ARb0r208c0m3@03
    w:ARb1r240c0m2@10 w:ARb1r208c0m4@30 w:ARb0r32c0m1@10 ARb1r0c1m0@01 F0b1r240c1 F0b1r240c0
    F0b1r208c0 F0b0r32c0 F0b0r160c1 O0b0r128c1 ARb0r128c1m1@03 w:ARb1r224c1m4@30 s:ARb1r64c0m0@03
    s:ARb1r96c0m0@03 s:ARb0r64c0m0@01 s:ARb1r208c0m0@03 s:ARb1r192c0m0@03 s:ARb1r224c0m0@03
    s:ARb0r96c0m0@01 ARb1r96c1m5@01 s:ARb0r32c0m0@01 s:ARb1r224c1m0@03 s:ARb1r128c1m0@03
    s:ARb1r208c1m0@01 s:ARb1r240c1m0@03 s:ARb0r96c1m2@01 s:ARb1r192c1m0@03 s:ARb0r64c1m0@01
    s:ARb1r160c0m0@03 s:ARb1r160c1m0@03 s:ARb0r32c1m0@01 s:ARb0r224c1m0@01 s:ARb0r160c0m0@01
    F0b0r240c0 F0b0r96c1 F0b0r128c1 F0b1r224c1 ARb0r128c0m3@01 w:ARb1r224c0m4@30
    w:ARb1r160c0m4@30 w:ARb0r208c1m0@10 s:ARb1r32c0m0@03 s:ARb1r32c1m0@03 s:ARb0r240c1m1@01
    s:ARb1r240c0m3@01 s:ARb1r128c0m0@03 s:ARb0r224c0m0@01 F0b1r160c1 F0b1r224c0 F0b1r160c0
    F0b1r64c1 ARb0r208c1m3@03 w:ARb1r32c0m4@30 F0b0r240c1 F0b1r32c0 ARb1r240c0m5@03
    w:ARb1r128c1m4@30 | s:ARb0r96c1m1@03 s:ARb0r240c0m0@01 s:ARb0r0c0m0@01 s:ARb0r208c1m1@01
    s:ARb0r192c1m1@01 s:ARb0r192c0m2@01 s:ARb0r160c1m3@03 F0b0r0c0 F0b1r128c1 ARb0r128c1m2@01
    w:ARb0r224c1m2@10 w:ARb0r192c1m0@10 ARb0r128c0m1@03 F0b1r96c1 F0b0r224c1 ARb0r192c1m3@03
    w:ARb1r32c1m4@30 s:ARb1r0c0m0@01 s:ARb1r64c1m1@03 s:ARb0r160c1m1@01 s:ARb1r96c1m1@03
    s:ARb0r240c1m3@03 F0b0r192c0 s:ARb0r208c0m3@03 F0b0r0c1 F0b1r32c1 ARb0r192c0m1@03
    w:ARb0r64c1m1@10 F0b0r192c1 s:ARb0r0c1m1@01 s:ARb0r208c0m1@01 s:ARb0r128c1m1@03
    s:ARb0r208c1m3@03 F0b0r224c0 F0b0r64c1 ARb0r0c1m3@03 w:ARb0r64c0m3@30 F0b1r96c0
    s:ARb1r64c1m5@01 s:ARb1r240c0m5@03 F0b1r64c0 F0b0r64c0 F0b0r128c0 F0b0r208c1 ARb1r0c1m2@03
    s:ARb0r128c0m1@03 F0b1r128c0 F0b1r0c1 F0b0r208c0 s:ARb1r0c1m0@01 s:ARb0r192c1m3@03 F0b0r160c0
    s:ARb0r192c0m1@03 F0b0r96c0 s:ARb1r96c1m5@01 s:ARb0r128c0m3@01 s:ARb0r128c1m2@01
    s:ARb0r0c1m3@03 s:ARb1r0c1m2@03 F0b1r208c1 F0b1r0c0
    """,
    """
    L1:Ka00 L1:Kt00 L1:Vt00 L1:Kt1z L1:Vt1z L1:Kt1a L1:Vt40 L1:Kt40 L1:xg L1:Vt1a L1:Vt57 L1:x0
    L1:Wq L1:VrA L1:KrZ L1:KrA L1:VrZ L1:Kt13 L1:Kt57 L1:Vt13 L1:x1 L1:Wo L1:KrM L1:VrM cKa00
    Ka00@10 cKt00 Kt00@10 cVt00 Vt00@10 cKVt51 KVt51@12 cKVt61 KVt61@10 w:L1:Kt1a s:Ka00@10
    cKVt40 s:Kt00@10 cKVt01 KVt40@12 cXg1 KVt01@10 cKVt11 s:Vt00@10 cX10 s:KVt51@12 Qg0j01@12
    s:KVt61@10 cWq2h0 cWq3h1 cWq2h1 cKVt31 cWq3h0 Q20Ld1 Q20L@10 K40x@12 Q30Ld1 Q20Td1 Q20T@10
    Q30Td1 s:KVt40@12 Wq7h2@10 Qg1 Qg1j01@12 w:L1:KrZ w:L1:KrA w:L1:VrA KVt11@10 s:KVt01@10
    GS1o3b1 GS1o0b1 cg0b1@12 w:L1:Kt13 cKVt60 s:Qg0j01@12 GS1o0b0 cKVt41 GS1o3b0 cg0b0@12
    KVt41@12 cKVt70 KVt60@10 w:K31@01 w:V31@01 s:Q20L@10 s:K40x@12 s:Q20T@10 s:Qg1j01@12 cX11
    Q21Ld1 Q21Td1 Q31Ld1 A31L Q31Td1 A31T cKVt50 cKVt71 cKVt21 cKVt20 w:L1:Wo w:K21@01 TR71T
    cWo2h0 cWo3h0 s:Wq7h2@10 s:cg0b1@12 s:cg0b0@12 A21T E1 cKVt10 CX71T@10 O1b1r192c0 cWo3h1
    O1b1r224c0 ARb1r224c0m1@12 ARb1r192c0m1@12 O1b1r160c0 A21L KVt10@10 ARb1r160c0m1@12 O1b1r32c0
    ARb1r32c0m1@12 w:Q70T@21 cKVt30 TR70T TR20T CX70T@10 ARb1r208c0m1@12 O1b1r96c0 cWo2h1
    O1b1r192c1 ARb1r192c1m1@12 O1b1r64c1 O1b1r96c1 ARb1r96c1m0@12 O1b1r224c1 ARb1r224c1m1@12
    ARb1r64c1m0@12 ARb1r240c1m1@12 O1b1r32c1 O1b1r160c1 ARb1r160c1m1@12 O1b1r128c1
    ARb1r128c1m1@12 w:K30@01 ARb1r96c0m1@12 s:KVt11@10 s:KVt41@12 s:KVt60@10 s:CX71T@10
    s:ARb1r224c0m1@12 s:ARb1r192c0m1@12 s:ARb1r160c0m1@12 s:ARb1r32c0m1@12 A30T A30L
    ARb1r32c1m1@12 w:C40L@21 w:Wo4h0@21 w:Wo5h0@21 w:Wo4h1@21 w:Wo5h1@21 s:ARb1r208c0m1@12
    s:ARb1r192c1m1@12 s:ARb1r96c1m0@12 s:ARb1r224c1m1@12 MG20L O1b0r32c0 O1b0r64c1 ARb0r64c1m1@10
    ARb1r240c0m2@10 O1b0r64c0 O1b1r64c0 ARb0r32c0m1@10 O1b0r32c1 ARb1r64c0m1@12 w:Q50T@21 MG20T
    TR50T O1b1r128c0 O1b0r96c1 ARb0r96c1m0@10 ARb0r32c1m1@10 w:ARb0r64c0m0@01 ARb1r128c0m1@12
    w:L1:KrM w:L1:VrM ARb0r64c0m1@12 MG50T GS1o1b0 O1b0r96c0 s:KVt10@10 s:CX70T@10
    s:ARb1r64c1m0@12 s:ARb1r240c1m1@12 O1b0r160c1 ARb0r160c1m0@10 w:ARb0r32c0m0@01 O1b0r128c1
    F1b0r32c0 O1b0r192c0 ARb0r208c0m0@10 ARb0r96c0m1@12 O1b0r192c1 O1b0r224c1 ARb0r240c1m0@10
    O1b0r160c0 ARb0r128c1m0@10 ARb1r208c1m2@12 ARb0r208c1m0@10 ARb0r32c0m2@12 GS1o2b0 O1b0r224c0
    ARb0r240c0m3@10 w:ARb0r64c1m0@01 ARb0r32c1m2@12 ARb0r64c1m2@12 ARb0r192c1m0@10
    s:ARb1r160c1m1@12 s:ARb1r128c1m1@12 s:ARb1r96c0m1@12 s:ARb1r32c1m1@12 ARb0r224c1m1@12
    ARb0r224c1m2@10 O1b0r128c0 ARb0r128c0m0@10 OG1b0 ARb0r0c0m1@10 ARb0r192c0m0@10
    ARb0r240c1m2@12 GS1o2b1 F1b0r32c1 ARb0r224c0m2@12 GS1o1b1 ARb0r240c0m1@12 ARb0r0c1m0@10
    w:ARb0r160c0m0@01 ARb0r224c0m1@10 ARb0r160c0m1@12 F1b0r160c0 OG1b1 F1b0r224c1 F1b1r208c0
    F1b0r240c1 F1b0r64c0 ARb1r0c1m1@10 F1b0r224c0 ARb0r192c1m2@12 F1b0r240c0 s:ARb0r64c1m1@10
    s:ARb1r240c0m2@10 s:ARb0r32c0m1@10 s:ARb1r64c0m1@12 s:ARb0r96c1m0@10 s:ARb0r32c1m1@10
    s:ARb1r128c0m1@12 s:ARb0r64c0m1@12 s:ARb0r160c1m0@10 s:ARb0r208c0m0@10 s:ARb0r96c0m1@12
    s:ARb0r240c1m0@10 s:ARb0r128c1m0@10 s:ARb1r208c1m2@12 s:ARb0r208c1m0@10 F1b1r64c0
    ARb0r160c0m2@10 ARb0r0c0m2@12 w:ARb0r96c1m2@01 w:ARb0r208c1m1@01 ARb1r0c0m1@10 F1b0r96c1
    F1b0r208c1 s:ARb0r32c0m2@12 s:ARb0r240c0m3@10 s:ARb0r32c1m2@12 s:ARb0r64c1m2@12
    s:ARb0r192c1m0@10 s:ARb0r224c1m1@12 s:ARb0r224c1m2@10 s:ARb0r128c0m0@10 s:ARb0r0c0m1@10
    s:ARb0r192c0m0@10 s:ARb0r240c1m2@12 s:ARb0r224c0m2@12 s:ARb0r240c0m1@12 F1b1r96c0 F1b0r0c0
    w:ARb0r192c0m2@01 ARb1r0c0m2@12 ARb0r192c0m3@12 w:ARb1r240c0m3@01 ARb0r208c1m2@12 F1b0r96c0
    ARb1r240c0m4@12 w:ARb1r208c1m3@21 F1b1r240c0 s:ARb0r0c1m0@10 s:ARb0r160c0m1@12 F1b0r160c1
    F1b1r208c1 F1b1r192c0 F1b1r0c0 s:ARb0r224c0m1@10 s:ARb0r192c1m2@12 F1b0r0c1 ARb0r160c1m2@12
    F1b1r224c0 ARb0r0c1m2@12 F1b0r192c1 s:ARb1r0c1m1@10 s:ARb0r0c0m2@12 ARb0r208c0m2@12
    w:ARb1r160c1m5@21 | F1b1r128c1 F1b0r192c0 F1b1r64c1 F1b0r208c0 F1b1r160c1 s:ARb0r160c0m2@10
    s:ARb1r0c0m1@10 s:ARb1r0c0m2@12 s:ARb0r192c0m3@12 F1b1r32c0 F1b1r0c1 ARb1r0c1m3@12
    w:ARb1r192c1m5@21 w:ARb1r224c1m5@21 w:ARb1r96c1m5@01 s:ARb0r208c1m2@12 s:ARb1r240c0m4@12
    F1b0r128c0 F1b1r192c1 w:ARb1r160c0m5@21 s:ARb0r160c1m2@12 s:ARb0r0c1m2@12 F1b1r32c1 F1b0r64c1
    F1b1r224c1 F1b1r160c0 F1b0r128c1 F1b1r96c1 s:ARb0r208c0m2@12 F1b1r128c0 s:ARb1r0c1m3@12
    F1b1r240c1
    """,
    """
    L2:Wq5h0 L2:Wo4h0 L2:Wq5h1 L2:Wq5h2 L2:x0 L2:xg L2:Wo4h1 L2:Wo5 L2:Ko0 L2:Vo3 L2:Vo0 L2:Vo1
    L2:Ko3 L2:Wq4 L2:Ko1 L2:Ko2 L2:Vo2 L2:x1 cWq5h0 Wq5h0@23 cWo4h0 Wo4h0@21 cWq5h1 Wq5h1@23
    cWq5h2 Wq5h2@23 cX20 Q50Td2 Q50T@21 cXg2 s:Wq5h0@23 cWo5h0 Wo5h0@23 cWo5h1 Wq7h2@21
    s:Wq5h1@23 Qg3j01@21 s:Wo4h0@21 KVt51@23 Q70T@21 s:Wq5h2@23 s:Q50T@21 Q71T@21 Wo5h1@21 E2
    s:Wq7h2@21 Qg0j01@23 Wo5h0@21 s:Wo5h0@23 s:Qg3j01@21 s:Q70T@21 cWq4h1 cWq4h0 Qg2 Qg2j0@23
    w:L2:Ko0 w:L2:Vo0 Q40Td2 GS2o0b1 w:L2:Wo4h1 Qg1j01@23 cWo4h1 Wo4h1@21 w:L2:Ko3 w:L2:Vo3
    GS2o0b0 GS2o3b0 GS2o3b1 w:K40@02 w:K40x@12 w:V40@02 w:KVt40@12 w:L2:Ko1 w:L2:Vo1 cg0b1@23
    A40T GS2o1b1 w:L2:Ko2 s:KVt51@23 cg0b0@23 GS2o2b0 Q40Ld2 A40L cX21 C40L@21 w:K41@02 Wo5h1@23
    GS2o1b0 Q41Td2 s:Q71T@21 s:Wo5h1@21 s:Qg0j01@23 s:Wo5h0@21 s:Qg2j0@23 s:Qg1j01@23 s:cg0b1@23
    A41T C50L@21 O2b1r224c0 O2b1r160c0 ARb1r240c0m0@21 w:ARb1r192c0m1@12 ARb1r224c0m3@23
    O2b1r192c0 O2b1r192c1 ARb1r192c0m3@23 s:Wo4h1@21 s:cg0b0@23 ARb1r160c0m3@23 O2b1r128c0 Q41Ld2
    s:C40L@21 CX50T@21 C40T@21 A41L O2b1r224c1 O2b1r32c0 O2b1r64c1 Qg2j01@21 w:ARb1r208c0m1@12
    ARb1r192c1m3@23 O2b1r96c1 ARb1r208c0m3@23 ARb1r32c0m3@23 s:Wo5h1@23 s:C50L@21
    s:ARb1r240c0m0@21 s:ARb1r224c0m3@23 ARb1r224c1m3@23 s:ARb1r192c0m3@23 ARb1r64c1m2@23 GS2o2b1
    w:ARb1r240c1m1@12 cg1b0@21 O2b1r128c1 ARb1r240c1m3@23 w:ARb1r160c1m1@12 ARb1r96c1m2@23
    O2b1r64c0 O2b1r96c0 O2b1r160c1 ARb1r160c1m3@23 ARb1r128c1m3@23 O2b1r32c1 w:ARb1r96c0m1@12
    s:ARb1r160c0m3@23 s:CX50T@21 s:C40T@21 s:ARb1r192c1m3@23 s:ARb1r208c0m3@23 s:ARb1r32c0m3@23
    s:ARb1r224c1m3@23 ARb1r32c1m3@23 ARb1r96c0m3@23 s:Qg2j01@21 s:ARb1r64c1m2@23
    s:ARb1r240c1m3@23 cg1b1@21 w:ARb1r208c0m2@32 s:ARb1r96c1m2@23 s:ARb1r160c1m3@23
    ARb0r64c0m2@23 w:ARb1r208c1m1@32 ARb1r208c0m5@21 w:ARb1r64c0m1@12 ARb1r208c1m3@21 F2b1r64c0
    ARb1r64c0m3@23 w:ARb1r128c0m1@12 ARb1r64c0m5@21 ARb1r128c0m3@23 s:cg1b0@21 s:ARb1r128c1m3@23
    ARb1r96c0m5@21 w:ARb1r192c0m2@32 ARb0r96c0m2@23 ARb1r192c0m5@21 s:ARb1r32c1m3@23
    ARb1r208c1m4@23 F2b0r64c0 F2b0r96c0 s:ARb1r96c0m3@23 ARb1r224c0m5@21 w:ARb1r224c1m2@32
    s:cg1b1@21 s:ARb0r64c0m2@23 s:ARb1r208c0m5@21 s:ARb1r208c1m3@21 ARb0r32c1m3@23
    w:ARb0r32c0m2@12 ARb1r224c1m5@21 ARb0r32c0m3@23 F2b1r224c1 F2b0r32c0 w:ARb1r160c1m2@32
    s:ARb1r64c0m3@23 F2b0r64c1 F2b1r208c0 ARb1r160c1m5@21 F2b1r160c1 F2b0r32c1 w:ARb1r128c1m2@32
    s:ARb1r64c0m5@21 s:ARb1r128c0m3@23 ARb0r224c1m3@23 s:ARb1r96c0m5@21 F2b0r240c1
    ARb1r128c1m5@21 w:ARb1r32c0m2@32 s:ARb0r96c0m2@23 s:ARb1r192c0m5@21 ARb0r224c0m3@23 F2b1r32c0
    F2b1r192c0 ARb1r32c0m5@21 s:ARb1r208c1m4@23 s:ARb1r224c0m5@21 F2b1r160c0 w:ARb1r192c1m2@32
    s:ARb1r224c1m5@21 ARb0r240c0m2@23 ARb1r192c1m5@21 ARb0r64c1m3@23 F2b0r224c0 F2b1r240c1
    F2b0r224c1 ARb1r160c0m5@21 s:ARb0r32c1m3@23 F2b0r160c0 s:ARb0r32c0m3@23 F2b1r32c1
    ARb0r160c0m3@23 ARb1r32c1m5@21 F2b1r208c1 s:ARb1r160c1m5@21 s:ARb0r224c1m3@23 ARb1r128c0m5@21
    F2b1r128c0 s:ARb1r128c1m5@21 s:ARb0r224c0m3@23 ARb0r0c0m3@23 ARb1r240c1m5@21 F2b0r0c0
    w:ARb0r96c1m3@32 w:ARb0r192c1m2@12 | s:ARb1r32c0m5@21 s:ARb0r240c0m2@23 ARb1r0c0m3@23
    F2b0r96c1 F2b1r0c0 F2b0r192c1 s:ARb1r192c1m5@21 s:ARb0r64c1m3@23 F2b0r192c0 F2b0r240c0
    s:ARb1r160c0m5@21 F2b0r208c1 F2b1r192c1 F2b1r96c0 F2b1r64c1 w:ARb1r96c1m3@32
    w:ARb1r240c0m4@12 s:ARb0r160c0m3@23 F2b0r160c1 w:ARb0r128c1m3@32 w:ARb0r0c1m2@12
    s:ARb1r32c1m5@21 s:ARb1r128c0m5@21 s:ARb0r0c0m3@23 F2b0r208c0 F2b0r128c0 F2b0r128c1 F2b0r0c1
    F2b1r224c0 F2b1r96c1 F2b1r128c1 s:ARb1r240c1m5@21 s:ARb1r0c0m3@23 F2b1r0c1 F2b1r240c0
    """,
    """
    L3:Wq6h0 L3:Wq6h1 L3:Wq6h2 L3:xg L3:Wq7 L3:Wq6h3 L3:x0 L3:x1 L3:Wo L3:Vo2 L3:Ko2 L3:Vo1
    L3:Vo3 L3:Ko1 L3:Ko3 L3:Ko0 L3:Vo0 cWq6h0 Wq6h0@30 cWq6h1 Wq6h1@30 cWq6h2 Wq6h2@30 cXg3
    cWq7h0 cWq7h2 Wq7h2@32 cWq6h3 cWq7h1 Wq6h3@30 Qg3 Qg3j01@32 s:Wq6h0@30 s:Wq6h1@30 cX30 Q70Td3
    Wq7h0@30 Q70T@32 cX31 Q71Td3 Q71T@32 Wq7h1@30 s:Wq6h2@30 s:Wq7h2@32 cWo7h1 cWo6h0 Wo6h0@30
    w:K50@03 w:V50@03 s:Qg3j01@32 Q50Td3 A50T cWo6h1 Q50Ld3 A50L Q51Ld3 cWo7h0 Wo7h0@30 Wo6h1@30
    w:L3:Ko2 w:L3:Vo2 Wo7h1@30 s:Wq6h3@30 s:Wq7h0@30 s:Q70T@32 s:Q71T@32 GS3o3b1 s:Wq7h1@30
    s:Wo6h0@30 GS3o2b1 C50L@32 Q51Td3 CX50T@32 w:Qg0j01@23 w:L3:Ko0 w:L3:Vo0 s:Wo7h0@30 GS3o1b1
    GS3o0b0 GS3o0b1 E3 GS3o1b0 GS3o3b0 cg0b1@30 GS3o2b0 cg1b0@32 w:KVt51@23 s:Wo6h1@30 s:C50L@32
    S51L S51T w:Wo5h0@23 cg0b0@30 s:Wo7h1@30 s:CX50T@32 A51Tb A51La A51Lb O3b1r224c0
    ARb1r240c0m1@30 w:ARb1r224c0m3@23 cg1b1@32 ARb1r224c0m4@30 A51Ta O3b1r192c0 w:Wo5h1@23
    ARb1r192c0m4@30 O3b1r160c0 O3b1r192c1 ARb1r160c0m4@30 O3b1r64c1 O3b1r64c0 O3b1r160c1
    O3b1r32c1 ARb1r208c1m1@32 w:ARb1r208c0m0@03 s:cg0b1@30 s:cg1b0@32 s:cg0b0@30 F3b1r192c0
    ARb1r208c0m2@32 ARb1r64c0m2@32 w:ARb1r192c1m3@23 ARb1r208c0m4@30 O3b1r32c0 ARb1r192c1m4@30
    ARb1r192c0m2@32 O3b1r224c1 O3b1r96c0 w:ARb1r96c0m0@03 ARb1r32c0m4@30 ARb1r96c0m2@32
    O3b1r128c1 ARb1r224c1m4@30 w:ARb1r224c1m0@03 s:ARb1r240c0m1@30 s:ARb1r224c0m4@30
    s:ARb1r192c0m4@30 ARb1r128c1m2@32 O3b1r96c1 ARb1r224c1m2@32 w:ARb1r224c0m0@03 O3b1r128c0
    ARb1r224c0m2@32 ARb1r64c1m4@30 s:cg1b1@32 s:ARb1r160c0m4@30 s:ARb1r208c1m1@32
    s:ARb1r208c0m4@30 F3b1r240c1 ARb1r240c1m4@30 F3b1r192c1 s:ARb1r208c0m2@32 s:ARb1r192c1m4@30
    ARb1r96c1m4@30 s:ARb1r64c0m2@32 s:ARb1r192c0m2@32 s:ARb1r32c0m4@30 ARb1r160c1m2@32
    s:ARb1r224c1m4@30 ARb1r160c1m4@30 ARb1r192c1m2@32 F3b1r224c1 s:ARb1r96c0m2@32
    s:ARb1r64c1m4@30 ARb1r128c1m4@30 F3b1r32c0 ARb1r32c0m2@32 ARb1r160c0m2@32 ARb1r240c1m2@32
    s:ARb1r128c1m2@32 s:ARb1r240c1m4@30 ARb1r32c1m4@30 ARb1r32c1m2@32 F3b1r160c1 F3b1r160c0
    s:ARb1r224c1m2@32 s:ARb1r224c0m2@32 s:ARb1r96c1m4@30 ARb1r96c0m4@30 w:ARb1r128c0m0@03
    s:ARb1r160c1m2@32 s:ARb1r160c1m4@30 ARb0r64c0m3@30 F3b0r96c1 ARb1r128c0m2@32 F3b1r208c0
    F3b0r64c0 s:ARb1r192c1m2@32 s:ARb1r128c1m4@30 ARb1r64c0m4@30 ARb0r96c1m3@32 s:ARb1r32c0m2@32
    s:ARb1r32c1m4@30 ARb1r128c0m4@30 F3b1r128c1 s:ARb1r160c0m2@32 s:ARb1r240c1m2@32
    s:ARb1r96c0m4@30 ARb0r96c0m3@30 w:ARb1r64c1m1@03 s:ARb1r32c1m2@32 s:ARb0r64c0m3@30
    ARb1r208c1m5@30 F3b0r208c0 ARb1r64c1m3@32 w:ARb0r240c1m3@03 w:ARb1r96c1m1@03 F3b1r224c0
    F3b0r240c1 s:ARb1r64c0m4@30 F3b0r128c1 ARb1r96c1m3@32 F3b1r208c1 F3b1r64c1 F3b0r32c1
    s:ARb1r128c0m2@32 s:ARb1r128c0m4@30 F3b0r208c1 F3b1r128c0 ARb0r128c1m3@32 s:ARb0r96c1m3@32
    F3b0r32c0 F3b0r96c0 | F3b0r224c1 w:ARb0r160c1m3@03 w:ARb1r240c0m5@03 s:ARb0r96c0m3@30
    ARb0r128c0m2@32 F3b0r160c1 F3b0r128c0 F3b1r96c0 w:ARb0r224c0m3@23 s:ARb1r208c1m5@30
    s:ARb1r64c1m3@32 F3b0r192c1 w:ARb0r240c0m2@23 F3b0r192c0 F3b1r240c0 s:ARb1r96c1m3@32
    F3b0r64c1 F3b1r96c1 F3b0r224c0 F3b1r32c1 F3b0r240c0 F3b0r0c1 F3b1r64c0 w:ARb0r160c0m3@23
    s:ARb0r128c1m3@32 F3b1r0c1 F3b0r160c0 s:ARb0r128c0m2@32 F3b0r0c0 F3b1r0c0
    """,
]


def _scores(q, kt):
    lo = lax.broadcasted_iota(jnp.int32, q.shape, 1) < 64
    zero = jnp.zeros_like(q)
    qs = jnp.concatenate([jnp.where(lo, q, zero), jnp.where(lo, zero, q)], axis=0)
    return jnp.dot(qs, kt, preferred_element_type=F32)


def _softmax(s, r0, k0):
    R, N = s.shape[0] // 2, s.shape[1]
    lane = lax.broadcasted_iota(jnp.int32, (R, 128), 1)
    lo = lane < 64
    tiles = []
    for t in range(N // 128):
        st = s[:, t * 128:(t + 1) * 128]
        kk = k0 + t * 128
        full = r0 + R <= 32 or (kk + 127 - r0 <= 128 and r0 + R - 1 - kk <= 128)
        if not full:
            qi = r0 + lax.broadcasted_iota(jnp.int32, (R, 128), 0)
            ki = kk + lane
            if kk > r0:
                keep = ki - qi <= 128
                if r0 < 32:
                    keep = keep | (qi < 32)
            else:
                keep = qi - ki <= 128
                if kk < 32:
                    keep = keep | (ki < 32)
            st = jnp.where(jnp.concatenate([keep, keep], axis=0), st, NEG)
        tiles.append(st)
    mx = tiles[0]
    for t in tiles[1:]:
        mx = jnp.maximum(mx, t)
    m = jnp.max(mx, axis=1, keepdims=True)
    ps = [jnp.exp2(t - m) for t in tiles]
    sm = ps[0]
    for t in ps[1:]:
        sm = sm + t
    l = jnp.sum(sm, axis=1, keepdims=True)
    p = jnp.concatenate([t.astype(BF16) for t in ps], axis=1)
    return p, jnp.where(lo, m[:R], m[R:]), jnp.where(lo, l[:R], l[R:])


def _values(p, l, vt):
    R = l.shape[0]
    c = lax.dot_general(p, vt, NT, preferred_element_type=F32)
    c = jnp.where(lax.broadcasted_iota(jnp.int32, (R, 128), 1) < 64, c[:R], c[R:])
    return c * pl.reciprocal(l, approx=False, full_range=False)


def _merge(parts):
    if len(parts) == 1:
        return parts[0]
    m = parts[0][1]
    for _, s in parts[1:]:
        m = jnp.maximum(m, s)
    ws = [jnp.exp2(s - m) for _, s in parts]
    den = ws[0]
    num = ws[0] * parts[0][0]
    for w, (c, _) in zip(ws[1:], parts[1:]):
        den = den + w
        num = num + w * c
    return num * pl.reciprocal(den, approx=False, full_range=False), m + jnp.log2(den)


def _pack(ctx, lse):
    ctx, lse = [jnp.concatenate([x[0:16], x[16:32]], axis=1) for x in (ctx, lse)]
    lane = lax.broadcasted_iota(jnp.int32, (16, 128), 1)
    s = lse[:, 0:128]
    for t in range(1, 8):
        s = jnp.where((lane % 64) // 8 == t, lse[:, t * 128:(t + 1) * 128], s)
    hi = s.astype(BF16).astype(F32)
    mid = (s - hi).astype(BF16).astype(F32)
    low = s - hi - mid
    k = lane % 8
    st = jnp.where(k == 0, hi, jnp.where(k == 1, mid, jnp.where(k == 2, low, 0.0)))
    return jnp.concatenate([ctx.astype(BF16), st.astype(BF16)], axis=1)


def _spread():
    r = lax.broadcasted_iota(jnp.int32, (128, 1024), 0)
    c = lax.broadcasted_iota(jnp.int32, (128, 1024), 1)
    pick = (r % 8 < 3) & (r // 64 == (c % 128) // 64) & ((r % 64) // 8 == c // 128)
    return jnp.where(pick, 1.0, 0.0).astype(BF16)


def _unpack(R, i):
    ref = R.grecv.at[i]
    lse = jnp.dot(ref[:, 1024:1152], R.spread[...], preferred_element_type=F32)
    ctx = jnp.concatenate([ref[:, 0:512], ref[:, 512:1024]], axis=0)
    return ctx.astype(F32), jnp.concatenate([lse[:, 0:512], lse[:, 512:1024]], axis=0)


def _side(ref, i):
    return jnp.concatenate([ref[i, t * 32:t * 32 + 32] for t in range(4)], axis=1)


def _stack(x):
    return jnp.concatenate([x[:, t * 128:t * 128 + 128] for t in range(4)], axis=0)


class _Task:
    def __init__(self, dev, kind, deps=(), run=None, copy=None, dst=None):
        self.dev, self.kind, self.deps = dev, kind, list(deps)
        self.run, self.copy, self.dst = run, copy, dst


def _slot(p, d):
    if p // 2 == d:
        return p % 2
    return 2 + [q for q in range(8) if d in [HOME[q]] + OUT[q] and q // 2 != d].index(p)


def _build():
    tasks, have, sl = {}, {}, slice
    count = {k: [0] * 4 for k in ("l", "s", "r", "ars", "arr", "gs", "gr", "t")}

    def nxt(kind, d):
        count[kind][d] += 1
        return count[kind][d] - 1

    def comp(name, d, deps, run, kind="comp"):
        tasks[name] = _Task(d, kind, deps, run)
        return [name]

    def send(name, u, v, deps, src, dst, prep=None):
        si, ri = nxt("s", u), nxt("r", v)

        def copy(R):
            return pltpu.make_async_remote_copy(
                src_ref=src(R), dst_ref=dst(R), send_sem=R.ssem.at[si], recv_sem=R.rsem.at[ri],
                device_id=(v,), device_id_type=MESH)
        name = "%s@%d%d" % (name, u, v)
        tasks[name] = _Task(u, "send", deps, prep, copy, v)
        return [name]

    def need(d, arrs, *box):
        return ["L%d:%s" % (d, n) for arr in arrs for n, a, *g in LOADS[d]
                if a == arr and all(x[0] < y[1] and y[0] < x[1] for x, y in zip(g, box))]

    for d in range(4):
        for name, arr, *box in LOADS[d]:
            def copy(R, arr=arr, idx=tuple(sl(*x) for x in box), i=nxt("l", d)):
                return pltpu.make_async_copy(R[arr].at[idx], R[arr + "s"].at[idx], R.lsem.at[i])
            tasks["L%d:%s" % (d, name)] = _Task(d, "load", copy=copy)

        def spread(R):
            R.spread[...] = _spread()

        def cxg(R):
            R.xb[:, 0:32, :] = R.xs[:, 0:32, :].astype(BF16)
        comp("E%d" % d, d, [], spread)
        comp("cXg%d" % d, d, need(d, ["x"], (0, 2), (0, 32)), cxg)
        for b in range(2):
            def cx(R, b=b):
                R.xb[b, 32:256, :] = R.xs[b, 32:256, :].astype(BF16)
            comp("cX%d%d" % (d, b), d, need(d, ["x"], (b, b + 1), (32, 256)), cx)

    for p in range(8):
        o, home = p // 2, HOME[p]
        cq = (p % 2 * 128, p % 2 * 128 + 128)
        for w, cuts, to in (("Wq", WQ_ROWS.get(p, (0, 256, 512)), {home}),
                            ("Wo", (0, 256, 512), set(OUT[p]))):
            for h in range(len(cuts) - 1):
                def at(R, z, w=w, rq=sl(cuts[h], cuts[h + 1]), buf="b"):
                    ref = R[w.lower() + buf]
                    return ref.at[rq, z:z + 128] if w == "Wq" else ref.at[z:z + 128, rq]

                def cast(R, at=at, z=cq[0]):
                    at(R, z)[...] = at(R, z, buf="s")[...].astype(BF16)
                nm = "%s%dh%d" % (w, p, h)
                box = (cuts[h], cuts[h + 1]), cq
                got = comp("c" + nm, o, need(o, [w.lower()], *(box if w == "Wq" else box[::-1])),
                           cast)
                key = (w, p) if w == "Wq" else (w, p, h)
                have.setdefault(key + (o,), []).extend(got)
                for v in sorted(to - {o}):
                    hop, z = got, cq[0]
                    for x, y in W_DETOUR.get(nm, [(o, v)]):
                        z1 = _slot(p, v) * 128 if y == v else 384
                        hop = send(nm, x, y, hop, lambda R, at=at, z=z: at(R, z),
                                   lambda R, at=at, z=z1: at(R, z))
                        z = z1
                    have.setdefault(key + (v,), []).extend(hop)

        for b in range(2):
            a, tri = MAIN[p][b], TRI[p][b]
            kv0, vlate = [], []
            for kv in range(2):
                nm = "%s%d%d" % ("KV"[kv], p, b)

                def ckv(R, b=b, p=p, kv=kv):
                    R.kvb[b, p, kv, :, 0:256] = (R.ks, R.vs)[kv][b, p].astype(BF16)
                got = comp("c" + nm, 0, need(0, "kv"[kv], (b, b + 1), (p, p + 1)), ckv)
                if a != 0:
                    cut, path = KV_DETOUR.get(nm, (128, ()))
                    cast, got = got, []
                    for x, r0, r1, hops in ((nm, 0, cut, [(0, a)]), (nm + "x", cut, 128, path)):
                        def ref(R, b=b, p=p, kv=kv, r0=r0, r1=r1):
                            return R.kvb.at[b, p, kv, r0:r1, 0:256]
                        hop = cast
                        for u, v in hops:
                            hop = send(x, u, v, hop, ref, ref)
                        got += hop if hops else []
                if kv and (p, b) in V_LAST:
                    vlate = got
                else:
                    kv0 += got
            kv1 = []
            pieces = [("KVt", 0, 2, 0, 128)]
            if (p, b) == FIRST_TRI:
                pieces = [("Ka", 0, 1, 0, 16), ("Kt", 0, 1, 16, 128), ("Vt", 1, 2, 0, 128)]
            for nm, k0, k1, r0, r1 in pieces:
                nm = "%s%d%d" % (nm, p, b)

                def ckt(R, b=b, p=p, k0=k0, k1=k1, r0=r0, r1=r1):
                    for kv in range(k0, k1):
                        R.kvb[b, p, kv, r0:r1, 256:384] = (
                            (R.ks, R.vs)[kv][b, p, r0:r1, 0:128].astype(BF16))
                got = comp("c" + nm, 1,
                           need(1, "kv"[k0:k1], (b, b + 1), (p, p + 1), (r0, r1), (0, 128)), ckt)
                if tri != 1:
                    def ref(R, b=b, p=p, k0=k0, k1=k1, r0=r0, r1=r1):
                        return R.kvb.at[b, p, k0:k1, r0:r1, 256:384]
                    for u, v in TRI_PATH.get((p, b), [(1, tri)]):
                        got = send(nm, u, v, got, ref, ref)
                kv1 += got

            for h, r0 in (("L", 0), ("T", 128)):
                tag = "%d%d%s" % (p, b, h)
                fin = MERGE_AT.get((p, b, h), home)
                cs = sl(_slot(p, fin) * 128, _slot(p, fin) * 128 + 128)

                def qproj(d, b=b, p=p, h=h, r0=r0, tag=tag):
                    z = _slot(p, d)

                    def run(R):
                        q = jnp.dot(R.xb[b, r0:r0 + 128], R.wqb[:, z * 128:z * 128 + 128],
                                    preferred_element_type=F32)
                        R.qb[b, p, r0:r0 + 128] = (q * SCALE).astype(BF16)
                    return comp("Q%sd%d" % (tag, d), d,
                                have["Wq", p, d] + ["cX%d%d" % (d, b)]
                                + (["cXg%d" % d] if h == "L" else []), run)
                qat = {home: qproj(home)}
                hops = [(home, a)] if a != home else []
                if h == "T" and tri not in (home, a):
                    hops += Q_TO_TRI[p]
                for u, v in hops:
                    if u not in qat:
                        qat[u] = qproj(u)

                    def ref(R, b=b, p=p, r0=r0):
                        return R.qb.at[b, p, r0:r0 + 128]
                    qat[v] = send("Q" + tag, u, v, qat[u], ref, ref)

                if h == "L":
                    jobs = [(a, 0, 256, kv0)]
                elif tri == a:
                    jobs = [(a, 0, 384, kv0 + kv1)]
                else:
                    jobs = [(a, 0, 256, kv0), (tri, 256, 384, kv1)]

                def put(R, c, lse, rr, b=b, cs=cs):
                    if rr == 0:
                        R.mctx[b, :, cs] = c[0:32]
                        R.mlse[b, :, cs] = lse[0:32]
                        c, rr = c[32:], 32
                    R.ctx[b, rr:rr + c.shape[0], cs] = c.astype(BF16)

                part = {}
                for d, k0, k1, ins in jobs:
                    ti = None if len(jobs) == 1 and d == fin else nxt("t", d)
                    late = vlate and not k0

                    def keep(R, c, m, l, rr, r0=r0, ti=ti, put=put):
                        if ti is None:
                            put(R, c, None if rr else m + jnp.log2(l), rr)
                        else:
                            R.tctx[ti, rr - r0:rr - r0 + 64] = c
                            R.tlse[ti, rr - r0:rr - r0 + 64] = m + jnp.log2(l)

                    def block(R, rr, b=b, p=p, k0=k0, k1=k1, keep=keep, late=late):
                        sc = _scores(R.qb[b, p, rr:rr + 64], R.kvb[b, p, 0, :, k0:k1])

                        def finish():
                            pr, m, l = _softmax(sc, rr, k0)
                            if late:
                                R.pb[rr // 64, :, 0:k1] = pr
                                R.pm[rr // 64] = m
                                R.pd[rr // 64] = l
                            else:
                                keep(R, _values(pr, l, R.kvb[b, p, 1, :, k0:k1]), m, l, rr)
                        return finish
                    got = comp(("TR" if k0 else "S" if late else "A") + tag, d, qat[d] + ins,
                               [lambda R, rr=rr, block=block: block(R, rr)
                                for rr in (r0, r0 + 64)], "blocks")
                    if late:
                        def rest(R, rr, b=b, p=p, k1=k1, keep=keep):
                            l = R.pd[rr // 64]
                            keep(R, _values(R.pb[rr // 64, :, 0:k1], l, R.kvb[b, p, 1, :, 0:k1]),
                                 R.pm[rr // 64], l, rr)
                        halves = [comp("A" + tag + "ab"[(rr - r0) // 64], d, got + vlate,
                                       lambda R, rr=rr, rest=rest: rest(R, rr))
                                  for rr in (r0, r0 + 64)]
                        got = halves[0] + halves[1]
                        if ti is None:
                            have["rows", p, b, r0 // 64] = halves[0]
                            have["rows", p, b, r0 // 64 + 1] = halves[1]
                    part[d] = (got, ti)
                if len(jobs) == 1 and a == fin:
                    have["ctx", p, b, h] = part[a][0]
                    continue

                deps, local = part.pop(fin, ([], None))
                (u0, (got, ti)), = part.items()
                si = nxt("gs", u0)

                def prep(R, si=si, ti=ti):
                    R.gsend[si] = _pack(_side(R.tctx, ti), _side(R.tlse, ti))

                def src(R, si=si):
                    return R.gsend.at[si]
                for u, v in BACK.get((p, b, h), [(u0, fin)]):
                    ri = nxt("gr", v)

                    def dst(R, ri=ri):
                        return R.grecv.at[ri]
                    got = send("CX" + tag, u, v, got, src, dst, prep)
                    src, prep = dst, None

                def mg(R, local=local, ri=ri, r0=r0, put=put):
                    parts = [] if local is None else [(R.tctx[local], R.tlse[local])]
                    parts.append(tuple(_stack(x) for x in _unpack(R, ri)))
                    put(R, *_merge(parts), r0)
                have["ctx", p, b, h] = comp("MG" + tag, fin, deps + got + ["E%d" % fin], mg)

    for p in range(8):
        for b in range(2):
            for h, r0, r1 in (("L", 32, 128), ("T", 128, 256)):
                got = have["ctx", p, b, h]
                for u, v in () if (p, b, h) in MERGE_AT else CTX_PATH.get((p, b), ()):
                    src, dst = [lambda R, b=b, r0=r0, r1=r1, z=_slot(p, d) * 128:
                                R.ctx.at[b, r0:r1, z:z + 128] for d in (u, v)]
                    got = send("C%d%d%s" % (p, b, h), u, v, got, src, dst)
                have["out", p, b, h] = got

    qg = {}
    for o in range(4):
        def qgp(R, o=o):
            xg = R.xb[:, 0:32, :].reshape(64, 512)
            q = jnp.dot(xg, R.wqb[:, 0:256], preferred_element_type=F32)
            R.qg[o] = (q * SCALE).astype(BF16)
        qg[o, o] = comp("Qg%d" % o, o,
                        ["cXg%d" % o] + have["Wq", 2 * o, o] + have["Wq", 2 * o + 1, o], qgp)
        for js, tree in QG_TREE[o]:
            def ref(R, o=o, js=js):
                return R.qg.at[o, :, js[0] * 128:js[-1] * 128 + 128]
            for u, v in tree:
                qg[o, v] = send("Qg%dj%s" % (o, "".join(map(str, js))), u, v, qg[o, u], ref, ref)
    for d in (1, 2, 3):
        for o in range(4):
            for b in range(2):
                def gs(R, p, o=o, b=b, d=d):
                    if HOME[p] == d != o:
                        q = R.qb[b, p, 0:32]
                    else:
                        q = R.qg[o, b * 32:b * 32 + 32, p % 2 * 128:p % 2 * 128 + 128]
                    sc = _scores(q, R.ks[b, p].astype(BF16))

                    def finish():
                        pr, m, l = _softmax(sc, 0, 256 * d)
                        R.gctx[b, p] = _values(pr, l, R.vs[b, p].astype(BF16))
                        R.glse[b, p] = m + jnp.log2(l)
                    return finish
                ps = (2 * o, 2 * o + 1)
                comp("GS%do%db%d" % (d, o, b), d,
                     qg[o, d] + [x for p in ps for x in need(d, "kv", (b, b + 1), (p, p + 1))]
                     + ["Q%d%dLd%d" % (p, b, d) for p in ps if HOME[p] == d != o],
                     [lambda R, p=p, gs=gs: gs(R, p) for p in ps], "blocks")

    def local(R, d, tiles):
        parts = []
        if d:
            parts.append([(R.gctx[b, p], R.glse[b, p]) for b, p in tiles])
        if any(HOME[p] == d for _, p in tiles):
            parts.append([(R.mctx[b, :, _slot(p, d) * 128:_slot(p, d) * 128 + 128],
                           R.mlse[b, :, _slot(p, d) * 128:_slot(p, d) * 128 + 128])
                          if HOME[p] == d else
                          (jnp.zeros((32, 128), F32), jnp.full((32, 128), -1e30, F32))
                          for b, p in tiles])
        return [tuple(jnp.concatenate(x, axis=1) for x in zip(*part)) for part in parts]

    def local_deps(d, tiles):
        return (sorted({"GS%do%db%d" % (d, p // 2, b) for b, p in tiles if d})
                + [x for b, p in tiles if HOME[p] == d for x in have["ctx", p, b, "L"]])

    for g in CG_PATH:
        for b in range(2):
            tiles = [(b, p) for p in range(8) if G_OUT[p] == g]
            got, ri = [], None
            for u, v in CG_PATH[g]:
                si, rn = nxt("gs", u), nxt("gr", v)

                def prep(R, u=u, si=si, ri=ri, tiles=tiles):
                    parts = local(R, u, tiles)
                    if ri is not None:
                        parts.append(_unpack(R, ri))
                    R.gsend[si] = _pack(*_merge(parts))
                got = send("cg%db%d" % (g, b), u, v,
                           got + (["E%d" % u] if got else []) + local_deps(u, tiles),
                           lambda R, si=si: R.gsend.at[si], lambda R, rn=rn: R.grecv.at[rn], prep)
                ri = rn

            def og(R, g=g, b=b, ri=ri, tiles=tiles):
                c, _ = _merge(local(R, g, tiles) + [_unpack(R, ri)])
                R.pacc[b, 0:32, :] = jnp.dot(c.astype(BF16), R.wob[...],
                                             preferred_element_type=F32)
            comp("OG%db%d" % (g, b), g,
                 got + ["E%d" % g] + local_deps(g, tiles)
                 + [x for _, p in tiles for h in range(2) for x in have["Wo", p, h, g]], og)

    for (b, r0, r1, c), pattern in ATOMS.items():
        msgs, final = PATTERNS[pattern]
        nm = "b%dr%dc%d" % (b, r0, c)
        rows, cols, n = sl(r0, r1), sl(c * 256, c * 256 + 256), r1 - r0
        own = {}
        for d in range(4):
            ps, ra = [p for p in range(8) if OUT[p][b] == d], r0 // 32 * 32
            own[d] = ["O%db%dr%dc%d" % (d, b, ra, c) if ra else "OG%db%d" % (d, b)]
            if ra and ps and own[d][0] not in tasks:
                ks = sl(_slot(ps[0], d) * 128, _slot(ps[-1], d) * 128 + 128)

                def op(R, b=b, ra=ra, ks=ks, cols=cols):
                    R.pacc[b, ra:ra + 32, cols] = jnp.dot(
                        R.ctx[b, ra:ra + 32, ks], R.wob[ks, cols], preferred_element_type=F32)
                comp(own[d][0], d,
                     [x for p in ps for x in have.get(
                         ("rows", p, b, r0 // 64), have["out", p, b, "LT"[r0 // 128]])]
                     + [x for p in ps for x in have["Wo", p, c, d]], op)

        def total(R, pieces, b=b, rows=rows, cols=cols, n=n):
            acc = None
            for x in pieces:
                v = R.pacc[b, rows, cols] if x is None else R.arr[x, 0:n].astype(F32)
                acc = v if acc is None else acc + v
            return acc
        names, slot = [], []
        for i, (u, v, cover) in enumerate(msgs):
            ri = nxt("arr", v)
            pieces = [None if x < 0 else slot[x] for x in cover]
            if pieces[0] is not None and len(pieces) == 1:
                prep, src = None, lambda R, x=pieces[0], n=n: R.arr.at[x, 0:n]
            else:
                si = nxt("ars", u)

                def prep(R, si=si, pieces=pieces, total=total, n=n):
                    R.ars[si, 0:n] = total(R, pieces).astype(BF16)

                def src(R, si=si, n=n):
                    return R.ars.at[si, 0:n]
            names += send("AR%sm%d" % (nm, i), u, v,
                          [y for x in cover for y in (own[u] if x < 0 else [names[x]])],
                          src, lambda R, ri=ri, n=n: R.arr.at[ri, 0:n], prep)
            slot.append(ri)
        for d in range(4):
            def fi(R, pieces=[None if x < 0 else slot[x] for x in final[d]], total=total, b=b,
                   rows=rows, cols=cols):
                R.out[b, rows, cols] = total(R, pieces)
            comp("F%d%s" % (d, nm), d,
                 [y for x in final[d] for y in (own[d] if x < 0 else [names[x]])], fi)
    return tasks, {k: max(v) for k, v in count.items()}


class _Refs(dict):
    __getattr__ = dict.__getitem__


def _signal(sem, to):
    pl.semaphore_signal(sem, inc=1, device_id=(to,), device_id_type=MESH)


def _prologue(d, R, tasks):
    bar = pltpu.get_barrier_semaphore()
    if d == 0:
        _signal(bar, 1)
        _signal(bar, 3)
    elif d != 2:
        _signal(bar, 0)
    loads = [name for name in ORDER[d].split() if name.startswith("L")]
    for name in loads[:2]:
        tasks[name].copy(R).start()
    if d % 2:
        pl.semaphore_wait(bar, 1)
        _signal(bar, 2)
    yield
    for name in loads[2:]:
        tasks[name].copy(R).start()
    if d == 2:
        pl.semaphore_wait(pltpu.get_barrier_semaphore(), 2)
        for v in (1, 3, 0):
            _signal(R.hsem, v)
    yield


def _program(d, R, tasks):
    waited, pending = set(), []
    known = set(((), (0,), (0, 1, 3), (0,))[d])

    def meet(v):
        if v in known:
            return
        if d == 0 and v != 2:
            pl.semaphore_wait(pltpu.get_barrier_semaphore(), 2)
            known.update((1, 3))
        else:
            pl.semaphore_wait(R.hsem, 1)
            known.update((2,) if d == 0 else (1, 2, 3))

    def flush(keep=0):
        while len(pending) > keep:
            pending.pop(0)[1]()

    def wait(name):
        t = tasks[name]
        if t.copy is None or name in waited:
            return
        flush()
        waited.add(name)
        if t.kind == "load":
            t.copy(R).wait()
        else:
            t.copy(R).wait_recv()

    for name in ORDER[d].split():
        if name == "|":
            flush()
            yield
        elif name.startswith("w:"):
            wait(name[2:])
        elif name.startswith("s:"):
            flush()
            tasks[name[2:]].copy(R).wait_send()
        elif not name.startswith("L"):
            t = tasks[name]
            for x in t.deps:
                wait(x)
            if any(n in t.deps for n, _ in pending):
                flush()
            if t.kind == "blocks":
                for block in t.run:
                    pending.append((name, block(R)))
                    flush(DEPTH)
            elif t.run is not None:
                t.run(R)
            if t.kind == "send":
                flush()
                meet(t.dst)
                t.copy(R).start()
    assert not pending and known | {d} == {0, 1, 2, 3}
    assert waited == {x for x, t in tasks.items() if t.copy and (t.dst, t.dev) in (
        (None, d), *((d, u) for u in range(4)))}
    assert sorted(x[2:] for x in ORDER[d].split() if x.startswith("s:")) == sorted(
        x for x, t in tasks.items() if t.kind == "send" and t.dev == d)
    yield


def pallas_dist_sparse_attn_localglobal_htp_kvseq_b2_sq256_skv256_hq4_dh64_kernel(
    x: jax.Array,
    Wq: jax.Array,
    K_ext: jax.Array,
    V_ext: jax.Array,
    Wo: jax.Array,
):
    kt = jnp.transpose(K_ext, (0, 2, 3, 1)).reshape(2, 8, 128, 256)
    vt = jnp.transpose(V_ext, (0, 2, 3, 1)).reshape(2, 8, 128, 256)
    tasks, n = _build()
    vmem, dma = pltpu.VMEM, pltpu.SemaphoreType.DMA
    scratch = dict(
        xs=vmem((2, 256, 512), F32), wqs=vmem((512, 256), F32), wos=vmem((256, 512), F32),
        ks=vmem((2, 8, 128, 256), F32), vs=vmem((2, 8, 128, 256), F32),
        xb=vmem((2, 256, 512), BF16), wqb=vmem((512, 512), BF16), wob=vmem((512, 512), BF16),
        kvb=vmem((2, 8, 2, 128, 384), BF16),
        qb=vmem((2, 8, 256, 128), BF16), qg=vmem((4, 64, 256), BF16),
        ctx=vmem((2, 256, 512), BF16),
        mctx=vmem((2, 32, 512), F32), mlse=vmem((2, 32, 512), F32),
        gctx=vmem((2, 8, 32, 128), F32), glse=vmem((2, 8, 32, 128), F32),
        gsend=vmem((n["gs"], 16, 1152), BF16), grecv=vmem((n["gr"], 16, 1152), BF16),
        spread=vmem((128, 1024), BF16),
        pb=vmem((4, 128, 384), BF16), pm=vmem((4, 64, 128), F32), pd=vmem((4, 64, 128), F32),
        tctx=vmem((n["t"], 128, 128), F32), tlse=vmem((n["t"], 128, 128), F32),
        pacc=vmem((2, 256, 512), F32),
        ars=vmem((n["ars"], 32, 256), BF16), arr=vmem((n["arr"], 32, 256), BF16),
        lsem=dma((n["l"],)), ssem=dma((n["s"],)), rsem=dma((n["r"],)),
        hsem=pltpu.SemaphoreType.REGULAR,
    )

    def body(x_ref, wq_ref, k_ref, v_ref, wo_ref, out_ref, *scr):
        R = _Refs(zip(scratch, scr), x=x_ref, wq=wq_ref, k=k_ref, v=v_ref, wo=wo_ref, out=out_ref)
        me = lax.axis_index("i")
        for emit in (_prologue, _program):
            stages = [emit(d, R, tasks) for d in range(4)]
            for _ in range(2):
                for d in CODE_ORDER:
                    pl.when(me == d)(lambda d=d: next(stages[d]))

    return pl.pallas_call(
        body,
        out_shape=jax.ShapeDtypeStruct(x.shape, F32),
        in_specs=[pl.BlockSpec(memory_space=pl.ANY)] * 5,
        out_specs=pl.BlockSpec(memory_space=pltpu.VMEM),
        scratch_shapes=list(scratch.values()),
        compiler_params=pltpu.CompilerParams(
            collective_id=0, vmem_limit_bytes=48 * 1024 * 1024,
            disable_bounds_checks=True, disable_semaphore_checks=True),
    )(x, Wq, kt, vt, Wo)
```
